```python
import numpy as np

kernel_name = "dist_layernorm_xy_m512_n256"

def setup_inputs():
    x = np.random.randn(1024, 512).astype(np.float32)
    gamma = np.random.randn(512).astype(np.float32)
    beta = np.random.randn(512).astype(np.float32)
    return {"x": x, "gamma": gamma, "beta": beta}

def reference(x: np.ndarray, gamma: np.ndarray, beta: np.ndarray) -> np.ndarray:
    eps = 1e-5
    mean = np.mean(x, axis=1, keepdims=True)
    var = np.var(x, axis=1, keepdims=True)
    return gamma * (x - mean) / np.sqrt(var + eps) + beta
```

```python
import jax
import jax.numpy as jnp
from jax import lax
from jax.experimental import pallas as pl
from jax.experimental.pallas import tpu as pltpu

EPS = 1e-5


def pallas_dist_layernorm_xy_m512_n256_kernel(
    x: jax.Array,
    gamma: jax.Array,
    beta: jax.Array,
):
    m, n = x.shape

    def body(x_ref, g_ref, b_ref, o_ref, mine, theirs, send_sem, recv_sem):
        my_x = lax.axis_index("x")
        my_y = lax.axis_index("y")
        peer = (my_x, 1 - my_y)
        barrier = pltpu.get_barrier_semaphore()
        pl.semaphore_signal(
            barrier, inc=1, device_id=peer, device_id_type=pl.DeviceIdType.MESH
        )
        xv = x_ref[...]
        mean = jnp.mean(xv, axis=1, keepdims=True)
        d = xv - mean
        m2 = jnp.sum(d * d, axis=1, keepdims=True)
        mine[0] = mean
        mine[1] = m2
        pl.semaphore_wait(barrier, 1)
        rdma = pltpu.make_async_remote_copy(
            mine, theirs, send_sem, recv_sem,
            device_id=peer, device_id_type=pl.DeviceIdType.MESH,
        )
        rdma.start()
        rdma.wait()
        mean_b = theirs[0]
        m2_b = theirs[1]
        delta = mean_b - mean
        mu = mean + 0.5 * delta
        var = (m2 + m2_b + delta * delta * (n / 2)) * (1.0 / (2 * n))
        rstd = lax.rsqrt(var + EPS)
        o_ref[...] = (xv - mu) * rstd * g_ref[...] + b_ref[...]

    return pl.pallas_call(
        body,
        out_shape=jax.ShapeDtypeStruct((m, n), x.dtype),
        in_specs=[pl.BlockSpec(memory_space=pltpu.VMEM)] * 3,
        out_specs=pl.BlockSpec(memory_space=pltpu.VMEM),
        scratch_shapes=[
            pltpu.VMEM((2, m, 1), jnp.float32),
            pltpu.VMEM((2, m, 1), jnp.float32),
            pltpu.SemaphoreType.DMA,
            pltpu.SemaphoreType.DMA,
        ],
        compiler_params=pltpu.CompilerParams(collective_id=0),
    )(x, gamma.reshape(1, n), beta.reshape(1, n))
```

```python
import math

import jax
import jax.numpy as jnp
from jax import lax
from jax.experimental import pallas as pl
from jax.experimental.pallas import tpu as pltpu

EPS = 1e-5
SUBLANES = 8

WHOLE, LEFT, RIGHT, SEND = "whole", "left", "right", "send"
AFTER_OUTPUT = "after output"

PLAN = (
    (WHOLE, 0, 128, 0),
    (LEFT, 128, 192, None),
    (SEND, 0, 128, None),
    (LEFT, 320, 176, 12),
    (RIGHT, 128, 48, 17),
    (RIGHT, 176, 48, 11),
    (RIGHT, 224, 48, 11),
    (RIGHT, 272, 48, None),
    (SEND, 128, 48, AFTER_OUTPUT),
    (RIGHT, 320, 48, 12),
    (SEND, 176, 48, 7),
    (RIGHT, 368, 48, 6),
    (SEND, 224, 48, 7),
    (RIGHT, 416, 32, None),
    (SEND, 272, 48, 7),
    (RIGHT, 448, 48, None),
    (SEND, 320, 64, 0),
    (SEND, 384, 48, 2),
    (SEND, 432, 64, 2),
)


def pallas_dist_layernorm_xy_m512_n256_kernel(
    x: jax.Array,
    gamma: jax.Array,
    beta: jax.Array,
):
    m, n = x.shape
    h = n // 2
    f32 = jnp.float32
    out_dtype = jnp.bfloat16

    loads = [step for step in PLAN if step[0] != SEND]
    sends = [step for step in PLAN if step[0] == SEND]
    cut = sum(rows for _, _, rows, _ in sends)
    raw = m - cut

    def body(x_hbm, gamma_hbm, beta_hbm, out_ref, whole_buf, left_buf, right_buf,
             raw_mine, raw_theirs, gamma_buf, beta_buf, load_sems, late_sems,
             send_sems, recv_sems, *stats_bufs):
        mine, theirs = stats_bufs[:len(sends)], stats_bufs[len(sends):]
        load_buf = {WHOLE: whole_buf, LEFT: left_buf, RIGHT: right_buf}

        def load(i):
            kind, start, rows, _ = loads[i]
            row_slice = pl.ds(start, rows)
            if kind == WHOLE:
                src = x_hbm.at[row_slice]
            else:
                src = x_hbm.at[row_slice, pl.ds(0 if kind == LEFT else h, h)]
            return pltpu.make_async_copy(
                src, load_buf[kind].at[row_slice], load_sems.at[i])

        for i in range(len(loads)):
            load(i).start()

        peer = (lax.axis_index("x"), 1 - lax.axis_index("y"))

        def remote(src, dst, k):
            return pltpu.make_async_remote_copy(
                src, dst, send_sems.at[k], recv_sems.at[k],
                device_id=peer, device_id_type=pl.DeviceIdType.MESH)

        def exchange(k):
            return remote(mine[k], theirs[k].at[0], k)

        barrier = pltpu.get_barrier_semaphore()
        pl.semaphore_signal(barrier, inc=1, device_id=peer,
                            device_id_type=pl.DeviceIdType.MESH)
        pl.semaphore_wait(barrier, 1)
        raw_rows = x_hbm.at[pl.ds(cut, raw)]
        forward = remote(raw_rows, raw_theirs, len(sends))
        forward.start()
        late_loads = [
            pltpu.make_async_copy(gamma_hbm, gamma_buf, late_sems.at[0]),
            pltpu.make_async_copy(beta_hbm, beta_buf, late_sems.at[1]),
            pltpu.make_async_copy(raw_rows, raw_mine, late_sems.at[2]),
        ]

        tile = (SUBLANES, h)
        diagonal = (lax.broadcasted_iota(jnp.int32, tile, 1)
                    - lax.broadcasted_iota(jnp.int32, tile, 0))

        def groups(start, rows):
            return range(start, start + rows, SUBLANES)

        def row_sum(v):
            return jnp.sum(v, axis=1, keepdims=True)

        def to_lanes(columns, start, rows):
            acc = jnp.zeros(tile, f32)
            for g in groups(start, rows):
                acc = jnp.where(diagonal == g - start, columns[g], acc)
            return jnp.sum(acc, axis=0, keepdims=True)

        def to_column(row, lane):
            spread = jnp.broadcast_to(row, tile)
            return row_sum(jnp.where(diagonal == lane, spread, 0.0))

        def hold_back(value, steps):
            for _ in range(steps):
                value = value * value
            return value

        pivot, mean, m2 = {}, {}, {}
        held = None
        n_loaded = n_sent = 0
        for kind, start, rows, hold in PLAN:
            if kind == SEND:
                mine[n_sent][0:1] = to_lanes(mean, start, rows)
                mine[n_sent][1:2] = to_lanes(m2, start, rows)
                exchange(n_sent).start()
                n_sent += 1
                continue

            if held is not None:
                spare = cut + SUBLANES * n_loaded
                load_buf[kind][spare:spare + SUBLANES, 0:h] = held
            load(n_loaded).wait()
            if n_loaded == len(loads) - 1:
                for copy in late_loads:
                    copy.start()
            n_loaded += 1
            for g in groups(start, rows):
                r = slice(g, g + SUBLANES)
                if kind == LEFT:
                    newest = left_buf[r]
                    pivot[g] = row_sum(newest) * (1.0 / h)
                elif kind == WHOLE:
                    a, b = whole_buf[r, 0:h], whole_buf[r, h:n]
                    mean[g] = row_sum(a + b) * (1.0 / n)
                    da, db = a - mean[g], b - mean[g]
                    newest = da * da + db * db
                    m2[g] = row_sum(newest)
                else:
                    a, b = left_buf[r], right_buf[r]
                    da, db = a - pivot[g], b - pivot[g]
                    newest = da * da + db * db
                    total = row_sum(da + db)
                    shift = total * (1.0 / n)
                    mean[g] = pivot[g] + shift
                    m2[g] = row_sum(newest) - total * shift
            held = None if hold is None else hold_back(newest, hold)

        for copy in late_loads:
            copy.wait()
        root = math.sqrt(2 * n)
        eps = 2 * n * EPS
        gamma_l = jnp.broadcast_to(gamma_buf[:, 0:h] * root, tile)
        gamma_r = jnp.broadcast_to(gamma_buf[:, h:n] * root, tile)
        beta_l = jnp.broadcast_to(beta_buf[:, 0:h], tile)
        beta_r = jnp.broadcast_to(beta_buf[:, h:n], tile)
        for k in range(len(sends)):
            exchange(k).wait_send()

        def halves(g):
            if g >= cut:
                r = slice(g - cut, g - cut + SUBLANES)
                return raw_mine[r, 0:h], raw_mine[r, h:n]
            r = slice(g, g + SUBLANES)
            if g in pivot:
                return left_buf[r], right_buf[r]
            return whole_buf[r, 0:h], whole_buf[r, h:n]

        norm = {}

        def write_rows(start, rows):
            for q in range(start, start + rows, 2 * SUBLANES):
                left, right = [], []
                for g in (q, q + SUBLANES):
                    mu, scale = norm[g]
                    a, b = halves(g)
                    left.append(((a - mu) * gamma_l) * scale + beta_l)
                    right.append(((b - mu) * gamma_r) * scale + beta_r)
                r = slice(q, q + 2 * SUBLANES)
                out_ref[r, 0:h] = jnp.concatenate(left, 0).astype(out_dtype)
                out_ref[r, h:n] = jnp.concatenate(right, 0).astype(out_dtype)
            return right[-1]

        forward.wait()
        for g in groups(cut, raw):
            r = slice(g - cut, g - cut + SUBLANES)
            parts = [*halves(g), raw_theirs[r, 0:h], raw_theirs[r, h:n]]
            mu = row_sum((parts[0] + parts[1]) + (parts[2] + parts[3])) * (0.5 / n)
            d = [p - mu for p in parts]
            squares = (d[0] * d[0] + d[1] * d[1]) + (d[2] * d[2] + d[3] * d[3])
            norm[g] = (mu, lax.rsqrt(row_sum(squares) + eps))
        write_rows(cut, raw)

        pending = []
        for k, (_, start, rows, hold) in enumerate(sends):
            if hold == AFTER_OUTPUT:
                theirs[k][1, 0:1] = write_rows(*pending.pop())[0:1]
            elif hold is not None:
                theirs[k][1, 0:1] = hold_back(scale, hold)
            exchange(k).wait_recv()
            my_mean, my_m2 = mine[k][0:1], mine[k][1:2]
            delta = theirs[k][0, 0:1] - my_mean
            mu = my_mean + 0.5 * delta
            scale = lax.rsqrt(((my_m2 + eps) + theirs[k][0, 1:2])
                              + (delta * (n / 2)) * delta)
            for g in groups(start, rows):
                norm[g] = (to_column(mu, g - start), to_column(scale, g - start))
            pending.append((start, rows))
        for start, rows in pending:
            write_rows(start, rows)

    buf_rows = cut + SUBLANES * len(loads)
    hbm = pl.BlockSpec(memory_space=pltpu.HBM)
    return pl.pallas_call(
        body,
        out_shape=jax.ShapeDtypeStruct((m, n), out_dtype),
        in_specs=[hbm, hbm, hbm],
        out_specs=pl.BlockSpec(memory_space=pltpu.VMEM),
        scratch_shapes=[
            pltpu.VMEM((buf_rows, n), f32),
            pltpu.VMEM((buf_rows, h), f32),
            pltpu.VMEM((buf_rows, h), f32),
            pltpu.VMEM((raw, n), f32),
            pltpu.VMEM((raw, n), f32),
            pltpu.VMEM((1, n), f32),
            pltpu.VMEM((1, n), f32),
            pltpu.SemaphoreType.DMA((len(loads),)),
            pltpu.SemaphoreType.DMA((3,)),
            pltpu.SemaphoreType.DMA((len(sends) + 1,)),
            pltpu.SemaphoreType.DMA((len(sends) + 1,)),
            *[pltpu.VMEM((2, h), f32) for _ in sends],
            *[pltpu.VMEM((2, 2, h), f32) for _ in sends],
        ],
        compiler_params=pltpu.CompilerParams(
            collective_id=0,
            disable_bounds_checks=True,
            disable_semaphore_checks=True,
            flags={"XLA_TPU_RESCHEDULE_DMA_DONES": True},
        ),
    )(x, gamma.reshape(1, n), beta.reshape(1, n))
```
